```python
import numpy as np

kernel_name = "dist_mean_ax0_shard0_i_m1024_n512"

def setup_inputs():
    return {"x": np.random.randn(4096, 512).astype(np.float32)}

def reference(x: np.ndarray) -> np.ndarray:
    return np.mean(x, axis=0, keepdims=True)
```

```python
import jax
import jax.numpy as jnp
from jax import lax
from jax.experimental import pallas as pl
from jax.experimental.pallas import tpu as pltpu

N_DEV = 4
SUBLANES = 8
CHUNKS = (944, 72, 8)
DIAGONAL = 2
PEERS = (DIAGONAL, 1, 3)


def _sum_row_tiles(ref, start, rows):
    accs = [None, None]
    for t in range(rows // SUBLANES):
        tile = ref[pl.ds(start + SUBLANES * t, SUBLANES), :]
        accs[t % 2] = tile if accs[t % 2] is None else accs[t % 2] + tile
    return accs[0] if accs[1] is None else accs[0] + accs[1]


def pallas_dist_mean_ax0_shard0_i_m1024_n512_kernel(x: jax.Array):
    m, n = x.shape
    assert sum(CHUNKS) == m
    starts = [sum(CHUNKS[:i]) for i in range(len(CHUNKS))]

    def kernel_body(x_hbm, out_ref, x_vmem, parts, load_sems, send_sems, recv_sems):
        loads = [
            pltpu.make_async_copy(
                x_hbm.at[pl.ds(start, rows)], x_vmem.at[pl.ds(start, rows)], load_sems.at[i]
            )
            for i, (start, rows) in enumerate(zip(starts, CHUNKS))
        ]
        for load in loads:
            load.start()

        me = lax.axis_index("i")
        barrier = pltpu.get_barrier_semaphore()
        sends = {}
        for d in PEERS:
            peer = (lax.rem(me + d, N_DEV),)
            pl.semaphore_signal(
                barrier, inc=1, device_id=peer, device_id_type=pl.DeviceIdType.MESH
            )
            sends[d] = pltpu.make_async_remote_copy(
                src_ref=parts.at[0],
                dst_ref=parts.at[d],
                send_sem=send_sems.at[d - 1],
                recv_sem=recv_sems.at[d - 1],
                device_id=peer,
                device_id_type=pl.DeviceIdType.MESH,
            )

        acc = None
        for i, (start, rows) in enumerate(zip(starts, CHUNKS)):
            loads[i].wait()
            part = _sum_row_tiles(x_vmem, start, rows)
            acc = part if acc is None else acc + part
            if i == 0:
                pl.semaphore_wait(barrier, N_DEV - 1)

        parts[0] = jnp.sum(acc, axis=0, keepdims=True) * (1.0 / (m * N_DEV))
        for d in PEERS:
            sends[d].start()
        for d in PEERS:
            sends[d].wait_send()

        sends[1].wait_recv()
        sends[3].wait_recv()
        total = parts[0] + parts[1] + parts[3]
        sends[DIAGONAL].wait_recv()
        out_ref[...] = total + parts[DIAGONAL]

    return pl.pallas_call(
        kernel_body,
        out_shape=pltpu.VMEM((1, n), x.dtype),
        in_specs=[pl.BlockSpec(memory_space=pltpu.HBM)],
        out_specs=pl.BlockSpec(memory_space=pltpu.VMEM),
        scratch_shapes=[
            pltpu.VMEM((m, n), x.dtype),
            pltpu.VMEM((N_DEV, 1, n), jnp.float32),
            pltpu.SemaphoreType.DMA((len(CHUNKS),)),
            pltpu.SemaphoreType.DMA((N_DEV - 1,)),
            pltpu.SemaphoreType.DMA((N_DEV - 1,)),
        ],
        compiler_params=pltpu.CompilerParams(
            collective_id=0,
            disable_bounds_checks=True,
            disable_semaphore_checks=True,
        ),
    )(x)
```

```python
from typing import NamedTuple

import jax
import jax.numpy as jnp
from jax import lax
from jax.experimental import pallas as pl
from jax.experimental.pallas import tpu as pltpu

N_DEV = 4
TILE_ROWS, TILE_COLS = 8, 128
ACCUMULATORS = 8

LEFT, DIAGONAL, RIGHT = 3, 2, 1


class Phase(NamedTuple):
    first: int
    steps: int
    col: int
    cols: int


EARLY_COLS = 384
ALL_COLUMNS = (Phase(0, 4, 0, 512), Phase(4, 36, 0, 512))
EARLY_COLUMNS = (Phase(40, 20, 0, 384), Phase(60, 4, 0, 384))
LATE_COLUMNS = (Phase(40, 20, 384, 128), Phase(60, 3, 384, 128), Phase(63, 1, 384, 128))
PHASES = ALL_COLUMNS + EARLY_COLUMNS + LATE_COLUMNS


def _start_load(x_hbm, phase, buf, sem):
    half = x_hbm.shape[0] // 2

    def start_step(i, carry=None):
        src_row = (phase.first + i) * TILE_ROWS
        dst_row = i * 2 * TILE_ROWS
        if not isinstance(i, int):
            src_row = pl.multiple_of(src_row, TILE_ROWS)
            dst_row = pl.multiple_of(dst_row, TILE_ROWS)
        for c in range(0, phase.cols, TILE_COLS):
            for h in range(2):
                pltpu.make_async_copy(
                    x_hbm.at[
                        pl.ds(src_row + h * half, TILE_ROWS),
                        pl.ds(phase.col + c, TILE_COLS),
                    ],
                    buf.at[
                        pl.ds(dst_row + h * TILE_ROWS, TILE_ROWS),
                        pl.ds(c, TILE_COLS),
                    ],
                    sem,
                ).start(priority=h)

    if phase.steps == 1:
        start_step(0)
    else:
        lax.fori_loop(0, phase.steps, start_step, None)


def _sum_tile_rows(buf):
    rows, cols = buf.shape
    sums = [None] * pl.cdiv(ACCUMULATORS, cols // TILE_COLS)
    for t in range(rows // TILE_ROWS):
        tile_row = buf[pl.ds(t * TILE_ROWS, TILE_ROWS), :]
        k = t % len(sums)
        sums[k] = tile_row if sums[k] is None else sums[k] + tile_row
    sums = [s for s in sums if s is not None]
    while len(sums) > 2:
        sums = sums[2:] + [sums[0] + sums[1]]
    return sums[0] if len(sums) == 1 else sums[0] + sums[1]


def pallas_dist_mean_ax0_shard0_i_m1024_n512_kernel(x: jax.Array):
    m, n = x.shape
    assert (m, n) == (1024, 512), "PHASES covers a (1024, 512) shard"
    scale = 1.0 / (m * N_DEV)

    def kernel_body(x_hbm, out_ref, bufs, mine, theirs, load_sems, send_sems, recv_sems):
        loads = {
            phase: (buf, load_sems.at[k])
            for k, (phase, buf) in enumerate(zip(PHASES, bufs, strict=True))
        }

        _start_load(x_hbm, PHASES[0], *loads[PHASES[0]])
        me = lax.axis_index("i")
        peers = {d: (lax.rem(me + d, N_DEV),) for d in (DIAGONAL, RIGHT, LEFT)}
        barrier = pltpu.get_barrier_semaphore()
        for peer in peers.values():
            pl.semaphore_signal(
                barrier, inc=1, device_id=peer, device_id_type=pl.DeviceIdType.MESH
            )
        for phase in PHASES[1:]:
            _start_load(x_hbm, phase, *loads[phase])

        def add_loaded(phases, acc=None):
            for phase in phases:
                buf, sem = loads[phase]
                pltpu.make_async_copy(buf, buf, sem).wait()
                part = _sum_tile_rows(buf)
                acc = part if acc is None else acc + part
            return acc

        def send(k, d, cols):
            copy = pltpu.make_async_remote_copy(
                src_ref=mine.at[:, cols],
                dst_ref=theirs.at[d - 1, :, cols],
                send_sem=send_sems.at[k],
                recv_sem=recv_sems.at[k],
                device_id=peers[d],
                device_id_type=pl.DeviceIdType.MESH,
            )
            copy.start()
            return copy

        early, late = pl.ds(0, EARLY_COLS), pl.ds(EARLY_COLS, n - EARLY_COLS)
        acc = add_loaded(ALL_COLUMNS)
        pl.semaphore_wait(barrier, N_DEV - 1)

        acc_early = add_loaded(EARLY_COLUMNS, acc[:, :EARLY_COLS])
        mine[:, early] = jnp.sum(acc_early, axis=0, keepdims=True) * scale
        diagonal_early = send(0, DIAGONAL, early)

        acc_late = add_loaded(LATE_COLUMNS, acc[:, EARLY_COLS:])
        mine[:, late] = jnp.sum(acc_late, axis=0, keepdims=True) * scale
        diagonal_late = send(1, DIAGONAL, late)
        right = send(2, RIGHT, pl.ds(0, n))
        left = send(3, LEFT, pl.ds(0, n))

        for copy in (diagonal_early, diagonal_late, right, left):
            copy.wait_send()
        right.wait_recv()
        left.wait_recv()
        neighbours = theirs[RIGHT - 1] + theirs[LEFT - 1]
        own = mine[...]
        diagonal_early.wait_recv()
        diagonal_late.wait_recv()
        out_ref[...] = (own + theirs[DIAGONAL - 1]) + neighbours

    return pl.pallas_call(
        kernel_body,
        out_shape=jax.ShapeDtypeStruct((1, n), jnp.float32),
        in_specs=[pl.BlockSpec(memory_space=pltpu.HBM)],
        out_specs=pl.BlockSpec(memory_space=pltpu.VMEM),
        scratch_shapes=[
            [pltpu.VMEM((2 * TILE_ROWS * p.steps, p.cols), x.dtype) for p in PHASES],
            pltpu.VMEM((1, n), jnp.float32),
            pltpu.VMEM((N_DEV - 1, 1, n), jnp.float32),
            pltpu.SemaphoreType.DMA((len(PHASES),)),
            pltpu.SemaphoreType.DMA((4,)),
            pltpu.SemaphoreType.DMA((4,)),
        ],
        compiler_params=pltpu.CompilerParams(
            collective_id=0,
            disable_bounds_checks=True,
            disable_semaphore_checks=True,
        ),
    )(x)
```

```python
from typing import NamedTuple

import jax
import jax.numpy as jnp
from jax import lax
from jax.experimental import pallas as pl
from jax.experimental.pallas import tpu as pltpu

N_DEV = 4
TILE_ROWS, TILE_COLS = 8, 128
ACCUMULATORS = 8

LEFT, DIAGONAL, RIGHT = 3, 2, 1


class Phase(NamedTuple):
    first: int
    steps: int
    col: int
    cols: int


EARLY_COLS = 384
ALL_COLUMNS = (Phase(0, 4, 0, 512), Phase(4, 36, 0, 512))
EARLY_COLUMNS = (Phase(40, 20, 0, 384), Phase(60, 4, 0, 384))
LATE_COLUMNS = (Phase(40, 20, 384, 128), Phase(60, 3, 384, 128), Phase(63, 1, 384, 128))
PHASES = ALL_COLUMNS + EARLY_COLUMNS + LATE_COLUMNS


def _start_load(x_hbm, phase, buf, sem):
    half = x_hbm.shape[0] // 2

    def start_step(i, carry=None):
        src_row = (phase.first + i) * TILE_ROWS
        dst_row = i * 2 * TILE_ROWS
        if not isinstance(i, int):
            src_row = pl.multiple_of(src_row, TILE_ROWS)
            dst_row = pl.multiple_of(dst_row, TILE_ROWS)
        for c in range(0, phase.cols, TILE_COLS):
            for h in range(2):
                pltpu.make_async_copy(
                    x_hbm.at[
                        pl.ds(src_row + h * half, TILE_ROWS),
                        pl.ds(phase.col + c, TILE_COLS),
                    ],
                    buf.at[
                        pl.ds(dst_row + h * TILE_ROWS, TILE_ROWS),
                        pl.ds(c, TILE_COLS),
                    ],
                    sem,
                ).start(priority=h)

    if phase.steps == 1:
        start_step(0)
    else:
        lax.fori_loop(0, phase.steps, start_step, None)


def _sum_tile_rows(buf):
    rows, cols = buf.shape
    sums = [None] * pl.cdiv(ACCUMULATORS, cols // TILE_COLS)
    for t in range(rows // TILE_ROWS):
        tile_row = buf[pl.ds(t * TILE_ROWS, TILE_ROWS), :]
        k = t % len(sums)
        sums[k] = tile_row if sums[k] is None else sums[k] + tile_row
    sums = [s for s in sums if s is not None]
    while len(sums) > 2:
        sums = sums[2:] + [sums[0] + sums[1]]
    return sums[0] if len(sums) == 1 else sums[0] + sums[1]


def pallas_dist_mean_ax0_shard0_i_m1024_n512_kernel(x: jax.Array):
    m, n = x.shape
    assert sorted(
        (p.first + i, p.col + c)
        for p in PHASES
        for i in range(p.steps)
        for c in range(0, p.cols, TILE_COLS)
    ) == [
        (i, c) for i in range(m // (2 * TILE_ROWS)) for c in range(0, n, TILE_COLS)
    ], "PHASES must load every tile of the shard exactly once"
    scale = 1.0 / (m * N_DEV)

    def kernel_body(x_hbm, out_ref, bufs, mine, theirs, load_sems, send_sems, recv_sems):
        loads = {
            phase: (buf, load_sems.at[k])
            for k, (phase, buf) in enumerate(zip(PHASES, bufs, strict=True))
        }

        _start_load(x_hbm, PHASES[0], *loads[PHASES[0]])
        me = lax.axis_index("i")
        peers = {d: (lax.rem(me + d, N_DEV),) for d in (DIAGONAL, RIGHT, LEFT)}
        barrier = pltpu.get_barrier_semaphore()
        for peer in peers.values():
            pl.semaphore_signal(
                barrier, inc=1, device_id=peer, device_id_type=pl.DeviceIdType.MESH
            )
        for phase in PHASES[1:]:
            _start_load(x_hbm, phase, *loads[phase])

        def add_loaded(phases, acc=None):
            for phase in phases:
                buf, sem = loads[phase]
                pltpu.make_async_copy(buf, buf, sem).wait()
                part = _sum_tile_rows(buf)
                acc = part if acc is None else acc + part
            return acc

        def send(k, d, cols):
            copy = pltpu.make_async_remote_copy(
                src_ref=mine.at[:, cols],
                dst_ref=theirs.at[d - 1, :, cols],
                send_sem=send_sems.at[k],
                recv_sem=recv_sems.at[k],
                device_id=peers[d],
                device_id_type=pl.DeviceIdType.MESH,
            )
            copy.start()
            return copy

        early, late = pl.ds(0, EARLY_COLS), pl.ds(EARLY_COLS, n - EARLY_COLS)
        acc = add_loaded(ALL_COLUMNS)
        pl.semaphore_wait(barrier, N_DEV - 1)

        acc_early = add_loaded(EARLY_COLUMNS, acc[:, :EARLY_COLS])
        mine[:, early] = jnp.sum(acc_early, axis=0, keepdims=True) * scale
        diagonal_early = send(0, DIAGONAL, early)

        acc_late = add_loaded(LATE_COLUMNS, acc[:, EARLY_COLS:])
        mine[:, late] = jnp.sum(acc_late, axis=0, keepdims=True) * scale
        diagonal_late = send(1, DIAGONAL, late)
        right = send(2, RIGHT, pl.ds(0, n))
        left = send(3, LEFT, pl.ds(0, n))

        for copy in (diagonal_early, diagonal_late, right, left):
            copy.wait_send()
        right.wait_recv()
        left.wait_recv()
        neighbours = theirs[RIGHT - 1] + theirs[LEFT - 1]
        own = mine[...]
        diagonal_early.wait_recv()
        diagonal_late.wait_recv()
        out_ref[...] = (own + theirs[DIAGONAL - 1]) + neighbours

    return pl.pallas_call(
        kernel_body,
        out_shape=jax.ShapeDtypeStruct((1, n), jnp.float32),
        in_specs=[pl.BlockSpec(memory_space=pltpu.HBM)],
        out_specs=pl.BlockSpec(memory_space=pltpu.VMEM),
        scratch_shapes=[
            [pltpu.VMEM((2 * TILE_ROWS * p.steps, p.cols), x.dtype) for p in PHASES],
            pltpu.VMEM((1, n), jnp.float32),
            pltpu.VMEM((N_DEV - 1, 1, n), jnp.float32),
            pltpu.SemaphoreType.DMA((len(PHASES),)),
            pltpu.SemaphoreType.DMA((4,)),
            pltpu.SemaphoreType.DMA((4,)),
        ],
        compiler_params=pltpu.CompilerParams(
            collective_id=0,
            disable_bounds_checks=True,
            disable_semaphore_checks=True,
        ),
    )(x)
```

```python
from typing import NamedTuple

import jax
import jax.numpy as jnp
from jax import lax
from jax.experimental import pallas as pl
from jax.experimental.pallas import tpu as pltpu

N_DEV = 4
TILE_ROWS, TILE_COLS = 8, 128
ACCUMULATORS = 8

LEFT, DIAGONAL, RIGHT = 3, 2, 1


class Phase(NamedTuple):
    starts: tuple[int, ...]
    steps: int
    col: int
    cols: int


EARLY_COLS = 384
ALL_COLUMNS = (
    Phase((0, 65), 4, 0, 512),
    Phase((4, 69), 37, 0, 512),
    Phase((41,), 2, 0, 512),
)
EARLY_COLUMNS = (
    Phase((43, 106), 18, 0, 384),
    Phase((61, 124), 4, 0, 384),
)
LATE_COLUMNS = (
    Phase((43, 106), 18, 384, 128),
    Phase((61, 124), 3, 384, 128),
    Phase((64, 127), 1, 384, 128),
)
PHASES = ALL_COLUMNS + EARLY_COLUMNS + LATE_COLUMNS


def _start_load(x_hbm, phase, buf, sem):
    def start_step(i, carry=None):
        for c in range(0, phase.cols, TILE_COLS):
            for h, start in enumerate(phase.starts):
                src_row = (start + i) * TILE_ROWS
                dst_row = (i * len(phase.starts) + h) * TILE_ROWS
                if not isinstance(i, int):
                    src_row = pl.multiple_of(src_row, TILE_ROWS)
                    dst_row = pl.multiple_of(dst_row, TILE_ROWS)
                pltpu.make_async_copy(
                    x_hbm.at[pl.ds(src_row, TILE_ROWS), pl.ds(phase.col + c, TILE_COLS)],
                    buf.at[pl.ds(dst_row, TILE_ROWS), pl.ds(c, TILE_COLS)],
                    sem,
                ).start(priority=h)

    if phase.steps == 1:
        start_step(0)
    else:
        lax.fori_loop(0, phase.steps, start_step, None)


def _sum_tile_rows(buf):
    rows, cols = buf.shape
    sums = [None] * pl.cdiv(ACCUMULATORS, cols // TILE_COLS)
    for t in range(rows // TILE_ROWS):
        tile_row = buf[pl.ds(t * TILE_ROWS, TILE_ROWS), :]
        k = t % len(sums)
        sums[k] = tile_row if sums[k] is None else sums[k] + tile_row
    sums = [s for s in sums if s is not None]
    while len(sums) > 2:
        sums = sums[2:] + [sums[0] + sums[1]]
    return sums[0] if len(sums) == 1 else sums[0] + sums[1]


def pallas_dist_mean_ax0_shard0_i_m1024_n512_kernel(x: jax.Array):
    m, n = x.shape
    assert sorted(
        (start + i, p.col + c)
        for p in PHASES
        for start in p.starts
        for i in range(p.steps)
        for c in range(0, p.cols, TILE_COLS)
    ) == [
        (r, c) for r in range(m // TILE_ROWS) for c in range(0, n, TILE_COLS)
    ], "PHASES must load every tile of the shard exactly once"
    scale = 1.0 / (m * N_DEV)

    def kernel_body(x_hbm, out_ref, bufs, mine, theirs, load_sems, send_sems, recv_sems):
        loads = {
            phase: (buf, load_sems.at[k])
            for k, (phase, buf) in enumerate(zip(PHASES, bufs, strict=True))
        }

        _start_load(x_hbm, PHASES[0], *loads[PHASES[0]])
        me = lax.axis_index("i")
        peers = {d: (lax.rem(me + d, N_DEV),) for d in (DIAGONAL, RIGHT, LEFT)}
        barrier = pltpu.get_barrier_semaphore()
        for peer in peers.values():
            pl.semaphore_signal(
                barrier, inc=1, device_id=peer, device_id_type=pl.DeviceIdType.MESH
            )
        for phase in PHASES[1:]:
            _start_load(x_hbm, phase, *loads[phase])

        def add_loaded(phases, acc=None):
            for phase in phases:
                buf, sem = loads[phase]
                pltpu.make_async_copy(buf, buf, sem).wait()
                part = _sum_tile_rows(buf)
                acc = part if acc is None else acc + part
            return acc

        def send(k, d, cols):
            copy = pltpu.make_async_remote_copy(
                src_ref=mine.at[:, cols],
                dst_ref=theirs.at[d - 1, :, cols],
                send_sem=send_sems.at[k],
                recv_sem=recv_sems.at[k],
                device_id=peers[d],
                device_id_type=pl.DeviceIdType.MESH,
            )
            copy.start()
            return copy

        early, late = pl.ds(0, EARLY_COLS), pl.ds(EARLY_COLS, n - EARLY_COLS)
        acc = add_loaded(ALL_COLUMNS)
        pl.semaphore_wait(barrier, N_DEV - 1)

        acc_early = add_loaded(EARLY_COLUMNS, acc[:, :EARLY_COLS])
        mine[:, early] = jnp.sum(acc_early, axis=0, keepdims=True) * scale
        diagonal_early = send(0, DIAGONAL, early)

        acc_late = add_loaded(LATE_COLUMNS, acc[:, EARLY_COLS:])
        mine[:, late] = jnp.sum(acc_late, axis=0, keepdims=True) * scale
        diagonal_late = send(1, DIAGONAL, late)
        right = send(2, RIGHT, pl.ds(0, n))
        left = send(3, LEFT, pl.ds(0, n))

        for copy in (diagonal_early, diagonal_late, right, left):
            copy.wait_send()
        right.wait_recv()
        left.wait_recv()
        neighbours = theirs[RIGHT - 1] + theirs[LEFT - 1]
        own = mine[...]
        diagonal_early.wait_recv()
        diagonal_late.wait_recv()
        out_ref[...] = (own + theirs[DIAGONAL - 1]) + neighbours

    return pl.pallas_call(
        kernel_body,
        out_shape=jax.ShapeDtypeStruct((1, n), jnp.float32),
        in_specs=[pl.BlockSpec(memory_space=pltpu.HBM)],
        out_specs=pl.BlockSpec(memory_space=pltpu.VMEM),
        scratch_shapes=[
            [
                pltpu.VMEM((len(p.starts) * p.steps * TILE_ROWS, p.cols), x.dtype)
                for p in PHASES
            ],
            pltpu.VMEM((1, n), jnp.float32),
            pltpu.VMEM((N_DEV - 1, 1, n), jnp.float32),
            pltpu.SemaphoreType.DMA((len(PHASES),)),
            pltpu.SemaphoreType.DMA((4,)),
            pltpu.SemaphoreType.DMA((4,)),
        ],
        compiler_params=pltpu.CompilerParams(
            collective_id=0,
            disable_bounds_checks=True,
            disable_semaphore_checks=True,
        ),
    )(x)
```
